```python
import numpy as np

kernel_name = "dist_sparse_attn_strided_htp_bs_b2_sq256_skv256_hq4_dh64"

def setup_inputs():
    x = np.random.randn(8, 256, 512).astype(np.float32)
    Wq = np.random.randn(512, 1024).astype(np.float32) * 0.02
    K_ext = np.random.randn(8, 256, 16, 64).astype(np.float32)
    V_ext = np.random.randn(8, 256, 16, 64).astype(np.float32)
    Wo = np.random.randn(1024, 512).astype(np.float32) * 0.02
    return {"x": x, "Wq": Wq, "K_ext": K_ext, "V_ext": V_ext, "Wo": Wo}

def reference(x, Wq, K_ext, V_ext, Wo):
    B, Sq, Skv, Hq, Dh = 8, 256, 256, 16, 64
    Q = (x @ Wq).reshape(B, Sq, Hq, Dh)
    qb = (np.arange(Sq) // 64)[:, None]
    kb = (np.arange(Skv) // 64)[None, :]
    mask = (qb == kb) | ((kb % 4) == (qb % 4))
    scores = np.einsum('bihd,bjhd->bhij', Q, K_ext).astype(np.float32) * 0.125
    scores = np.where(mask[None, None, :, :], scores, -1e9)
    scores_max = scores.max(axis=-1, keepdims=True)
    w = np.exp(scores - scores_max)
    row_keep = mask.any(axis=1)
    w_sum = np.where(row_keep[None, None, :, None], w.sum(axis=-1, keepdims=True), 1.0)
    w = w / w_sum
    w = np.where(row_keep[None, None, :, None], w, 0.0)
    ctx = np.einsum('bhij,bjhd->bihd', w, V_ext).reshape(B, Sq, Hq * Dh)
    return ctx @ Wo
```

```python
import functools
import jax
import jax.numpy as jnp
from jax import lax
from jax.experimental import pallas as pl
from jax.experimental.pallas import tpu as pltpu

N_DEV = 4
B_LOC = 2
SQ = 256
DM = 512
BLK = 64
T = B_LOC * SQ
LOG2E = 1.4426950408889634
QSCALE = 0.125 * LOG2E
MESH = pl.DeviceIdType.MESH
SCOPES = False
WO0 = 1024
RAMP = (32, 96, 384)

def scope(name):
    if SCOPES:
        return jax.named_scope(name)
    import contextlib
    return contextlib.nullcontext()


def wo_row(par, c, hh):
    return WO0 + par * 512 + c * 128 + hh * 64


def pallas_dist_sparse_attn_strided_htp_bs_b2_sq256_skv256_hq4_dh64_kernel(x, Wq, K_ext, V_ext, Wo):
    bf16 = jnp.bfloat16
    f32 = jnp.float32
    x2 = x.reshape(T, DM)
    kt = jnp.transpose(K_ext, (0, 2, 3, 1)).reshape(8, 8, 128, SQ)
    vt = jnp.transpose(V_ext, (0, 2, 3, 1)).reshape(8, 8, 128, SQ)
    NR = len(RAMP)
    roff = [sum(RAMP[:i]) for i in range(NR)]
    FWD_O = ((0, 128), (128, 128), (256, 128), (384, 64), (448, 64))
    NP = NR + 1 + 1 + 1 + 2 + len(FWD_O)

    def body(x_hbm, wq_hbm, kt_hbm, vt_hbm, wo_hbm, out_ref,
             x_f, x_b, wq_f, wo_f, w_all, k_v, v_v, ctx,
             lsem, ksem, vsem, ssem, rsem, fsem, rdy):
        me = lax.axis_index("i")
        left = (me + 3) % N_DEV
        right = (me + 1) % N_DEV
        diag = (me + 2) % N_DEV
        slot_dev = [me, left, right, diag]
        nfence = [0]

        def fence():
            pl.semaphore_signal(fsem, 1)
            nfence[0] += 1

        with scope("issue"):
            ld_wq = [pltpu.make_async_copy(wq_hbm.at[roff[i]:roff[i] + RAMP[i], :],
                                           wq_f.at[roff[i]:roff[i] + RAMP[i], :], lsem.at[i]) for i in range(NR)]
            ld_x = pltpu.make_async_copy(x_hbm, x_f, lsem.at[NR])
            ld_wo = pltpu.make_async_copy(wo_hbm, wo_f, lsem.at[NR + 1])
            pair_order = [(0, 0), (0, 1), (1, 0), (2, 1), (1, 1), (2, 0), (3, 0), (3, 1)]
            ld_k, ld_v = {}, {}
            for (s, h) in pair_order:
                p = 2 * s + h
                g = 2 * slot_dev[s] + h
                ld_k[(s, h)] = pltpu.make_async_copy(kt_hbm.at[pl.ds(2 * me, 2), g], k_v.at[p], ksem.at[p])
                ld_v[(s, h)] = pltpu.make_async_copy(vt_hbm.at[pl.ds(2 * me, 2), g], v_v.at[p], vsem.at[p])
            for i in range(NR):
                ld_wq[i].start()
                fence()
            bar = pltpu.get_barrier_semaphore()

            @pl.when(me < 2)
            def _():
                pl.semaphore_signal(bar, inc=1, device_id=(right,), device_id_type=MESH)

            @pl.when((me == 0) | (me == 3))
            def _():
                pl.semaphore_signal(bar, inc=1, device_id=(left,), device_id_type=MESH)

            fence()
            ld_x.start()
            fence()
            ld_wo.start()
            fence()
            for sh in pair_order:
                ld_k[sh].start(); ld_v[sh].start()

        with scope("bar"):
            @pl.when(me == 2)
            def _():
                pl.semaphore_wait(bar, 2)

            @pl.when(me % 2 == 1)
            def _():
                pl.semaphore_wait(bar, 1)

            early = [me >= 2, (me == 1) | (me == 2)]

            @pl.when(early[0])
            def _():
                pl.semaphore_signal(rdy.at[1], inc=1, device_id=(right,), device_id_type=MESH)

            @pl.when(early[1])
            def _():
                pl.semaphore_signal(rdy.at[0], inc=1, device_id=(left,), device_id_type=MESH)

        def rdma(ssl, dsl, r0, n, idx, dev):
            return pltpu.make_async_remote_copy(w_all.at[ssl, r0:r0 + n], w_all.at[dsl, r0:r0 + n],
                                                ssem.at[idx], rsem.at[idx],
                                                device_id=(dev,), device_id_type=MESH)

        def mk(d):
            dev = right if d == 0 else left
            sl = 1 if d == 0 else 2
            q0 = 0 if d == 0 else 512
            q1 = 512 - q0
            o0 = WO0 + q0
            o1 = WO0 + q1
            specs = {}
            for i in range(NR):
                specs[("qa", i)] = (0, sl, q0 + roff[i], RAMP[i])
            specs["qb"] = (0, sl, q1, 512)
            specs["oa"] = (0, sl, o0, 512)
            specs["fq"] = (sl, 3, q0, 512)
            specs[("ob", 0)] = (0, sl, o1, 256)
            specs[("ob", 1)] = (0, sl, o1 + 256, 256)
            for i, (r, n) in enumerate(FWD_O):
                specs[("fo", i)] = (sl, 3, o0 + r, n)
            assert len(specs) == NP
            return {k: rdma(*v, d * NP + i, dev) for i, (k, v) in enumerate(specs.items())}
        cp = [mk(0), mk(1)]

        for i in range(NR):
            with scope(f"wq{i}"):
                ld_wq[i].wait()
                for h in range(2):
                    w_all[0, 512 * h + roff[i]:512 * h + roff[i] + RAMP[i], :] = (
                        wq_f[roff[i]:roff[i] + RAMP[i], 128 * h:128 * (h + 1)].astype(bf16))
                for d in range(2):
                    @pl.when(early[d])
                    def _():
                        cp[d][("qa", i)].start()
                        if i == NR - 1:
                            cp[d]["qb"].start()
        with scope("late"):
            for d in range(2):
                @pl.when(jnp.logical_not(early[d]))
                def _():
                    pl.semaphore_wait(rdy.at[d], 1)
                    for i in range(NR):
                        cp[d][("qa", i)].start()
                    cp[d]["qb"].start()
        with scope("x"):
            ld_x.wait()
            x_b[...] = x_f[...].astype(bf16)

        lo = lax.broadcasted_iota(jnp.int32, (T, 128), 1) < 64
        r2 = lax.broadcasted_iota(jnp.int32, (128, 128), 0) < 64
        l2 = lax.broadcasted_iota(jnp.int32, (128, 128), 1) < 64
        m_diag = r2 == l2
        ones_d = jnp.where(m_diag, 1.0, 0.0).astype(bf16)
        ones_a = jnp.where(m_diag, 0.0, 1.0).astype(bf16)

        def prep(w):
            w = jnp.concatenate([w[0:64], pltpu.roll(w[64:128], 64, 1)], axis=0)
            return (jnp.where(m_diag, w, 0.0).astype(bf16), jnp.where(m_diag, 0.0, w).astype(bf16))

        def attn(pairs):
            for sh in pairs:
                ld_k[sh].wait(); ld_v[sh].wait()
            qs = []
            for (s, h) in pairs:
                q = jnp.dot(x_b[...], w_all[s, 512 * h:512 * (h + 1), :], preferred_element_type=f32)
                qs.append((q * QSCALE).astype(bf16))
            scs = []
            for (s, h), q in zip(pairs, qs):
                p = 2 * s + h
                blocks = []
                for b in range(B_LOC):
                    for t in range(2):
                        wk = prep(k_v[p, b, :, 128 * t:128 * (t + 1)])
                        for j in range(2):
                            r0 = b * SQ + t * 128 + j * BLK
                            blocks.append(jnp.dot(q[r0:r0 + BLK], wk[j], preferred_element_type=f32))
                scs.append(jnp.concatenate(blocks, axis=0))
            pes = []
            for sc in scs:
                m0 = jnp.max(jnp.where(lo, sc, -jnp.inf), axis=1, keepdims=True)
                m1 = jnp.max(jnp.where(lo, -jnp.inf, sc), axis=1, keepdims=True)
                pes.append(jnp.exp2(sc - jnp.where(lo, m0, m1)).astype(bf16))
            for (s, h), pe in zip(pairs, pes):
                p = 2 * s + h
                for b in range(B_LOC):
                    for t in range(2):
                        wv = prep(v_v[p, b, :, 128 * t:128 * (t + 1)])
                        for j in range(2):
                            r0 = b * SQ + t * 128 + j * BLK
                            pb = pe[r0:r0 + BLK]
                            l = jnp.dot(pb, ones_d if j == 0 else ones_a, preferred_element_type=f32)
                            o = lax.dot_general(pb, wv[j], (((1,), (1,)), ((), ())), preferred_element_type=f32)
                            r = pl.reciprocal(l, approx=True)
                            r = r * (2.0 - l * r)
                            ctx[r0:r0 + BLK, 128 * p:128 * (p + 1)] = (o * r).astype(bf16)

        def wo_tile(s, c, hh):
            return jnp.concatenate([w_all[s, wo_row(0, c, hh):wo_row(0, c, hh) + 64, :],
                                    w_all[s, wo_row(1, c, hh):wo_row(1, c, hh) + 64, :]], axis=0)

        def oproj(tiles, c, first, msplit=1):
            m = T // msplit
            for mi in range(msplit):
                rows = slice(mi * m, (mi + 1) * m)
                acc = None
                for (s, hh) in tiles:
                    p = 2 * s + hh
                    d = jnp.dot(ctx[rows, 128 * p:128 * (p + 1)], wo_tile(s, c, hh), preferred_element_type=f32)
                    acc = d if acc is None else acc + d
                if first:
                    out_ref[rows, 128 * c:128 * (c + 1)] = acc
                else:
                    out_ref[rows, 128 * c:128 * (c + 1)] += acc

        with scope("wo"):
            ld_wo.wait()
            for par in range(2):
                for c in range(4):
                    for hh in range(2):
                        h = 2 * hh + par
                        w_all[0, wo_row(par, c, hh):wo_row(par, c, hh) + 64, :] = (
                            wo_f[64 * h:64 * (h + 1), 128 * c:128 * (c + 1)].astype(bf16))
            cp[0]["oa"].start(); cp[1]["oa"].start()
        with scope("a0"):
            attn([(0, 0), (0, 1)])
        with scope("r1"):
            for d in range(2):
                for i in range(NR):
                    cp[d][("qa", i)].wait_recv()
                cp[d]["fq"].start(); cp[d][("ob", 0)].start(); cp[d][("ob", 1)].start()
        with scope("a1"):
            attn([(1, 0), (2, 1)])
        with scope("r2"):
            cp[0]["qb"].wait_recv(); cp[1]["qb"].wait_recv()
        with scope("a2"):
            attn([(1, 1), (2, 0)])
        with scope("o0"):
            for c in range(4):
                oproj([(0, 0), (0, 1)], c, True)
        with scope("r3"):
            for d in range(2):
                cp[d]["oa"].wait_recv()
                for i in range(len(FWD_O)):
                    cp[d][("fo", i)].start()
        with scope("r4"):
            cp[0]["fq"].wait_recv(); cp[1]["fq"].wait_recv()
        with scope("a3"):
            attn([(3, 0), (3, 1)])
        for i in range(2):
            with scope(f"r5{i}"):
                cp[0][("ob", i)].wait_recv(); cp[1][("ob", i)].wait_recv()
            with scope(f"o2{i}"):
                for c in (2 * i, 2 * i + 1):
                    oproj([(1, 0), (1, 1), (2, 0), (2, 1)], c, False)
        for i in range(3):
            with scope(f"r6{i}"):
                cp[0][("fo", i)].wait_recv(); cp[1][("fo", i)].wait_recv()
            with scope(f"o3{i}"):
                oproj([(3, 0), (3, 1)], i, False, msplit=2)
        with scope("r63"):
            cp[0][("fo", 3)].wait_recv(); cp[1][("fo", 3)].wait_recv()
        with scope("o33"):
            oproj([(3, 0)], 3, False, msplit=4)
        with scope("sw0"):
            pl.semaphore_wait(fsem, nfence[0])
            for d in range(2):
                for k, c in cp[d].items():
                    if k[0] != "fo":
                        c.wait_send()
        with scope("r64"):
            cp[0][("fo", 4)].wait_recv(); cp[1][("fo", 4)].wait_recv()
        with scope("o34"):
            oproj([(3, 1)], 3, False, msplit=4)
        with scope("sw"):
            for d in range(2):
                for k, c in cp[d].items():
                    if k[0] == "fo":
                        c.wait_send()

    out = pl.pallas_call(
        body,
        out_shape=jax.ShapeDtypeStruct((T, DM), f32),
        in_specs=[pl.BlockSpec(memory_space=pl.ANY)] * 5,
        out_specs=pl.BlockSpec(memory_space=pltpu.VMEM),
        scratch_shapes=[
            pltpu.VMEM((T, DM), f32),
            pltpu.VMEM((T, DM), bf16),
            pltpu.VMEM((DM, 256), f32),
            pltpu.VMEM((256, DM), f32),
            pltpu.VMEM((4, 2048, 128), bf16),
            pltpu.VMEM((8, 2, 128, SQ), f32),
            pltpu.VMEM((8, 2, 128, SQ), f32),
            pltpu.VMEM((T, 1024), bf16),
            pltpu.SemaphoreType.DMA((NR + 2,)),
            pltpu.SemaphoreType.DMA((8,)),
            pltpu.SemaphoreType.DMA((8,)),
            pltpu.SemaphoreType.DMA((2 * NP,)),
            pltpu.SemaphoreType.DMA((2 * NP,)),
            pltpu.SemaphoreType.REGULAR,
            pltpu.SemaphoreType.REGULAR((2,)),
        ],
        compiler_params=pltpu.CompilerParams(collective_id=0, disable_semaphore_checks=True,
                                             vmem_limit_bytes=64 * 1024 * 1024),
    )(x2, Wq, kt, vt, Wo)
    return out.reshape(B_LOC, SQ, DM)
```

```python
import jax
import jax.numpy as jnp
from jax import lax
from jax.experimental import pallas as pl
from jax.experimental.pallas import tpu as pltpu

B_LOC = 2
SQ = 256
DM = 512
BLK = 64
T = B_LOC * SQ
QSCALE = 0.125 * 1.4426950408889634
MESH = pl.DeviceIdType.MESH
WO0 = 1024
F32ROWS = 32
RAMP = (48, 64, 160, 208)
FWD_O = ((0, 128), (128, 128), (256, 128), (384, 64), (448, 64))


def _wo_row(par, c, hh):
    return WO0 + par * 512 + c * 128 + hh * 64


def pallas_dist_sparse_attn_strided_htp_bs_b2_sq256_skv256_hq4_dh64_kernel(x, Wq, K_ext, V_ext, Wo):
    bf16 = jnp.bfloat16
    f32 = jnp.float32
    n_b, _, n_h, _ = K_ext.shape
    x2 = x.reshape(T, DM)
    kt = jnp.transpose(K_ext, (0, 2, 3, 1)).reshape(n_b, n_h // 2, 128, SQ)
    vt = jnp.transpose(V_ext, (0, 2, 3, 1)).reshape(n_b, n_h // 2, 128, SQ)

    NR = len(RAMP)
    NF = len(FWD_O)
    assert F32ROWS + sum(RAMP) == DM
    roff = [sum(RAMP[:i]) for i in range(NR)]
    F0 = DM - F32ROWS
    lrows = list(RAMP[:-1]) + [RAMP[-1] + F32ROWS]
    NP = NR + NF + 6
    pair_order = [(0, 0), (0, 1), (1, 0), (2, 1), (1, 1), (2, 0), (3, 0), (3, 1)]

    def body(x_hbm, wq_hbm, kt_hbm, vt_hbm, wo_hbm, out_ref,
             x_f, x_b, wq_f, wo_f, w_all, head_f, k_v, v_v, ctx,
             lsem, ksem, vsem, ssem, rsem, fsem, rdy):
        me = lax.axis_index("i")
        left = (me + 3) & 3
        right = (me + 1) & 3
        diag = (me + 2) & 3
        slot_dev = [me, left, right, diag]
        n_fence = [0]

        def fence():
            pl.semaphore_signal(fsem, 1)
            n_fence[0] += 1

        def make_copies(d):
            dev = right if d == 0 else left
            sl = 1 + d
            qa, qb = 512 * d, 512 * (1 - d)
            oa, ob = WO0 + qa, WO0 + qb
            specs = {("qa", i): (0, sl, qa + roff[i], RAMP[i]) for i in range(NR)}
            specs[("qb", 0)] = (0, sl, qb, 512)
            specs[("oa", 0)] = (0, sl, oa, 512)
            specs[("fq", 0)] = (sl, 3, qa, 512)
            specs[("ob", 0)] = (0, sl, ob, 256)
            specs[("ob", 1)] = (0, sl, ob + 256, 256)
            for i, (r, n) in enumerate(FWD_O):
                specs[("fo", i)] = (sl, 3, oa + r, n)
            refs = {k: (w_all.at[s0, r:r + n], w_all.at[s1, r:r + n]) for k, (s0, s1, r, n) in specs.items()}
            refs[("hd", 0)] = (wq_hbm.at[F0:DM, 128 * d:128 * (d + 1)], head_f.at[d])
            assert len(refs) == NP
            return {k: pltpu.make_async_remote_copy(src, dst, ssem.at[d * NP + i], rsem.at[d * NP + i],
                                                    device_id=(dev,), device_id_type=MESH)
                    for i, (k, (src, dst)) in enumerate(refs.items())}

        cp = [make_copies(0), make_copies(1)]

        def wait_recv(name, i=0):
            cp[0][(name, i)].wait_recv()
            cp[1][(name, i)].wait_recv()

        def wait_send(name, i=0):
            cp[0][(name, i)].wait_send()
            cp[1][(name, i)].wait_send()

        ld_wq = [pltpu.make_async_copy(wq_hbm.at[roff[i]:roff[i] + lrows[i], :],
                                       wq_f.at[roff[i]:roff[i] + lrows[i], :], lsem.at[i]) for i in range(NR)]
        ld_x = pltpu.make_async_copy(x_hbm, x_f, lsem.at[NR])
        ld_wo = pltpu.make_async_copy(wo_hbm, wo_f, lsem.at[NR + 1])
        ld_k, ld_v = {}, {}
        for (s, h) in pair_order:
            p = 2 * s + h
            g = 2 * slot_dev[s] + h
            ld_k[(s, h)] = pltpu.make_async_copy(kt_hbm.at[pl.ds(B_LOC * me, B_LOC), g], k_v.at[p], ksem.at[p])
            ld_v[(s, h)] = pltpu.make_async_copy(vt_hbm.at[pl.ds(B_LOC * me, B_LOC), g], v_v.at[p], vsem.at[p])

        early = [me >= 2, (me == 1) | (me == 2)]
        bar = pltpu.get_barrier_semaphore()

        ld_wq[0].start()
        for d, pos in ((1, 1), (0, 3)):
            @pl.when(me == pos)
            def _():
                pl.semaphore_wait(bar, 1)
                cp[d][("hd", 0)].start()
                pl.semaphore_signal(rdy.at[1 - d], inc=1, device_id=(0,), device_id_type=MESH)
                pl.semaphore_signal(bar, inc=1, device_id=(2,), device_id_type=MESH)

        @pl.when(me == 0)
        def _():
            pl.semaphore_signal(bar, inc=1, device_id=(1,), device_id_type=MESH)
            pl.semaphore_signal(bar, inc=1, device_id=(3,), device_id_type=MESH)

        for ld in ld_wq[1:] + [ld_x, ld_wo]:
            fence()
            ld.start()
        for sh in pair_order:
            fence()
            ld_k[sh].start()
            ld_v[sh].start()

        @pl.when(me == 2)
        def _():
            pl.semaphore_wait(bar, 2)
            cp[0][("hd", 0)].start()
            cp[1][("hd", 0)].start()
            pl.semaphore_signal(rdy.at[1], inc=1, device_id=(3,), device_id_type=MESH)
            pl.semaphore_signal(rdy.at[0], inc=1, device_id=(1,), device_id_type=MESH)

        for i in range(NR):
            ld_wq[i].wait()
            for h in range(2):
                w_all[0, 512 * h + roff[i]:512 * h + roff[i] + lrows[i], :] = (
                    wq_f[roff[i]:roff[i] + lrows[i], 128 * h:128 * (h + 1)].astype(bf16))
            for d in range(2):
                @pl.when(early[d])
                def _():
                    cp[d][("qa", i)].start()
                    if i == NR - 1:
                        cp[d][("qb", 0)].start()
        for d in range(2):
            @pl.when(jnp.logical_not(early[d]))
            def _():
                pl.semaphore_wait(rdy.at[d], 1)
                for i in range(NR):
                    cp[d][("qa", i)].start()
                cp[d][("hd", 0)].start()
                cp[d][("qb", 0)].start()

        ld_x.wait()
        x_b[...] = x_f[...].astype(bf16)
        ld_wo.wait()
        for par in range(2):
            for c in range(4):
                for hh in range(2):
                    h = 2 * hh + par
                    w_all[0, _wo_row(par, c, hh):_wo_row(par, c, hh) + 64, :] = (
                        wo_f[64 * h:64 * (h + 1), 128 * c:128 * (c + 1)].astype(bf16))
        cp[0][("oa", 0)].start()
        cp[1][("oa", 0)].start()

        lo = lax.broadcasted_iota(jnp.int32, (T, 128), 1) < BLK
        m_diag = ((lax.broadcasted_iota(jnp.int32, (128, 128), 0) < BLK)
                  == (lax.broadcasted_iota(jnp.int32, (128, 128), 1) < BLK))
        seg_sum = (jnp.where(m_diag, 1.0, 0.0).astype(bf16), jnp.where(m_diag, 0.0, 1.0).astype(bf16))

        def block_weights(w):
            w = jnp.concatenate([w[0:BLK], pltpu.roll(w[BLK:128], BLK, 1)], axis=0)
            return jnp.where(m_diag, w, 0.0).astype(bf16), jnp.where(m_diag, 0.0, w).astype(bf16)

        def attn(pairs):
            for sh in pairs:
                ld_k[sh].wait()
                ld_v[sh].wait()
            qs = []
            for (s, h) in pairs:
                q = jnp.dot(x_b[...], w_all[s, 512 * h:512 * (h + 1), :], preferred_element_type=f32)
                qs.append((q * QSCALE).astype(bf16))
            scores = []
            for (s, h), q in zip(pairs, qs):
                blocks = []
                for b in range(B_LOC):
                    for t in range(2):
                        wk = block_weights(k_v[2 * s + h, b, :, 128 * t:128 * (t + 1)])
                        for j in range(2):
                            r0 = b * SQ + t * 128 + j * BLK
                            blocks.append(jnp.dot(q[r0:r0 + BLK], wk[j], preferred_element_type=f32))
                scores.append(jnp.concatenate(blocks, axis=0))
            probs = []
            for sc in scores:
                m0 = jnp.max(jnp.where(lo, sc, -jnp.inf), axis=1, keepdims=True)
                m1 = jnp.max(jnp.where(lo, -jnp.inf, sc), axis=1, keepdims=True)
                probs.append(jnp.exp2(sc - jnp.where(lo, m0, m1)).astype(bf16))
            for (s, h), pe in zip(pairs, probs):
                p = 2 * s + h
                for b in range(B_LOC):
                    for t in range(2):
                        wv = block_weights(v_v[p, b, :, 128 * t:128 * (t + 1)])
                        for j in range(2):
                            r0 = b * SQ + t * 128 + j * BLK
                            pb = pe[r0:r0 + BLK]
                            l = jnp.dot(pb, seg_sum[j], preferred_element_type=f32)
                            o = lax.dot_general(pb, wv[j], (((1,), (1,)), ((), ())),
                                                preferred_element_type=f32)
                            r = pl.reciprocal(l, approx=True)
                            r = r * (2.0 - l * r)
                            ctx[r0:r0 + BLK, 128 * p:128 * (p + 1)] = (o * r).astype(bf16)

        def oproj(pairs, c, first=False, msplit=1):
            m = T // msplit
            for mi in range(msplit):
                rows = slice(mi * m, (mi + 1) * m)
                acc = None
                for (s, hh) in pairs:
                    p = 2 * s + hh
                    w = jnp.concatenate([w_all[s, _wo_row(par, c, hh):_wo_row(par, c, hh) + 64, :]
                                         for par in range(2)], axis=0)
                    d = jnp.dot(ctx[rows, 128 * p:128 * (p + 1)], w, preferred_element_type=f32)
                    acc = d if acc is None else acc + d
                if first:
                    out_ref[rows, 128 * c:128 * (c + 1)] = acc
                else:
                    out_ref[rows, 128 * c:128 * (c + 1)] += acc

        attn(pair_order[0:2])
        for d in range(2):
            cp[d][("hd", 0)].wait_recv()
            w_all[1 + d, 512 * d + F0:512 * d + DM, :] = head_f[d].astype(bf16)
            for i in range(NR):
                cp[d][("qa", i)].wait_recv()
            cp[d][("fq", 0)].start()
            cp[d][("ob", 0)].start()
            cp[d][("ob", 1)].start()
        attn(pair_order[2:4])
        wait_recv("qb")
        attn(pair_order[4:6])
        for c in range(4):
            oproj([(0, 0), (0, 1)], c, first=True)
        for d in range(2):
            cp[d][("oa", 0)].wait_recv()
            for i in range(NF):
                cp[d][("fo", i)].start()
        pl.semaphore_wait(fsem, n_fence[0])
        wait_send("hd")
        for i in range(NR):
            wait_send("qa", i)
        wait_send("qb")
        wait_send("oa")
        wait_recv("fq")
        attn(pair_order[6:8])
        for i in range(2):
            wait_recv("ob", i)
            for c in (2 * i, 2 * i + 1):
                oproj([(1, 0), (1, 1), (2, 0), (2, 1)], c)
        wait_send("fq")
        wait_send("ob", 0)
        wait_send("ob", 1)
        for i in range(NF):
            wait_send("fo", i)
            wait_recv("fo", i)
            if i < 3:
                oproj([(3, 0), (3, 1)], i, msplit=2)
            else:
                oproj([(3, i - 3)], 3, msplit=4)

    out = pl.pallas_call(
        body,
        out_shape=jax.ShapeDtypeStruct((T, DM), f32),
        in_specs=[pl.BlockSpec(memory_space=pl.ANY)] * 5,
        out_specs=pl.BlockSpec(memory_space=pltpu.VMEM),
        scratch_shapes=[
            pltpu.VMEM((T, DM), f32),
            pltpu.VMEM((T, DM), bf16),
            pltpu.VMEM((DM, 256), f32),
            pltpu.VMEM((256, DM), f32),
            pltpu.VMEM((4, 2048, 128), bf16),
            pltpu.VMEM((2, F32ROWS, 128), f32),
            pltpu.VMEM((8, B_LOC, 128, SQ), f32),
            pltpu.VMEM((8, B_LOC, 128, SQ), f32),
            pltpu.VMEM((T, 1024), bf16),
            pltpu.SemaphoreType.DMA((NR + 2,)),
            pltpu.SemaphoreType.DMA((8,)),
            pltpu.SemaphoreType.DMA((8,)),
            pltpu.SemaphoreType.DMA((2 * NP,)),
            pltpu.SemaphoreType.DMA((2 * NP,)),
            pltpu.SemaphoreType.REGULAR,
            pltpu.SemaphoreType.REGULAR((2,)),
        ],
        compiler_params=pltpu.CompilerParams(collective_id=0, disable_semaphore_checks=True,
                                             vmem_limit_bytes=32 * 1024 * 1024),
    )(x2, Wq, kt, vt, Wo)
    return out.reshape(B_LOC, SQ, DM)
```

```python
import jax
import jax.numpy as jnp
from jax import lax
from jax.experimental import pallas as pl
from jax.experimental.pallas import tpu as pltpu

B_LOC = 2
SQ = 256
DM = 512
BLK = 64
T = B_LOC * SQ
QSCALE = 0.125 * 1.4426950408889634
MASKED = -1e9 * 1.4426950408889634
MESH = pl.DeviceIdType.MESH
WO0 = 1024
F32ROWS = 32
RAMP = (48, 48, 112, 272)
FWD_O = ((0, 128), (128, 128), (256, 128), (384, 64), (448, 64))


def _wo_row(par, c, hh):
    return WO0 + par * 512 + c * 128 + hh * 64


def pallas_dist_sparse_attn_strided_htp_bs_b2_sq256_skv256_hq4_dh64_kernel(x, Wq, K_ext, V_ext, Wo):
    bf16 = jnp.bfloat16
    f32 = jnp.float32
    n_b, _, n_h, _ = K_ext.shape
    x2 = x.reshape(T, DM)
    kt = jnp.transpose(K_ext, (0, 2, 3, 1)).reshape(n_b, n_h // 2, 128, SQ)
    vt = jnp.transpose(V_ext, (0, 2, 3, 1)).reshape(n_b, n_h // 2, 128, SQ)

    NR = len(RAMP)
    NF = len(FWD_O)
    assert F32ROWS + sum(RAMP) == DM
    roff = [sum(RAMP[:i]) for i in range(NR)]
    F0 = DM - F32ROWS
    lrows = list(RAMP[:-1]) + [RAMP[-1] + F32ROWS]
    NP = NR + NF + 6
    pair_order = [(0, 0), (0, 1), (1, 0), (2, 1), (1, 1), (2, 0), (3, 0), (3, 1)]

    def body(x_hbm, wq_hbm, kt_hbm, vt_hbm, wo_hbm, out_ref,
             x_f, x_b, wq_f, wo_f, w_all, head_f, k_v, v_v, ctx,
             lsem, ksem, vsem, ssem, rsem, fsem, rdy):
        me = lax.axis_index("i")
        left = (me + 3) & 3
        right = (me + 1) & 3
        diag = (me + 2) & 3
        slot_dev = [me, left, right, diag]
        n_fence = [0]

        def fence():
            pl.semaphore_signal(fsem, 1)
            n_fence[0] += 1

        def make_copies(d):
            dev = right if d == 0 else left
            sl = 1 + d
            qa, qb = 512 * d, 512 * (1 - d)
            oa, ob = WO0 + qa, WO0 + qb
            specs = {("qa", i): (0, sl, qa + roff[i], RAMP[i]) for i in range(NR)}
            specs[("qb", 0)] = (0, sl, qb, 512)
            specs[("oa", 0)] = (0, sl, oa, 512)
            specs[("fq", 0)] = (sl, 3, qa, 512)
            specs[("ob", 0)] = (0, sl, ob, 256)
            specs[("ob", 1)] = (0, sl, ob + 256, 256)
            for i, (r, n) in enumerate(FWD_O):
                specs[("fo", i)] = (sl, 3, oa + r, n)
            refs = {k: (w_all.at[s0, r:r + n], w_all.at[s1, r:r + n]) for k, (s0, s1, r, n) in specs.items()}
            refs[("hd", 0)] = (wq_hbm.at[F0:DM, 128 * d:128 * (d + 1)], head_f.at[d])
            assert len(refs) == NP
            return {k: pltpu.make_async_remote_copy(src, dst, ssem.at[d * NP + i], rsem.at[d * NP + i],
                                                    device_id=(dev,), device_id_type=MESH)
                    for i, (k, (src, dst)) in enumerate(refs.items())}

        cp = [make_copies(0), make_copies(1)]

        def wait_recv(name, i=0):
            cp[0][(name, i)].wait_recv()
            cp[1][(name, i)].wait_recv()

        def wait_send(name, i=0):
            cp[0][(name, i)].wait_send()
            cp[1][(name, i)].wait_send()

        ld_wq = [pltpu.make_async_copy(wq_hbm.at[roff[i]:roff[i] + lrows[i], :],
                                       wq_f.at[roff[i]:roff[i] + lrows[i], :], lsem.at[i]) for i in range(NR)]
        ld_x = pltpu.make_async_copy(x_hbm, x_f, lsem.at[NR])
        ld_wo = pltpu.make_async_copy(wo_hbm, wo_f, lsem.at[NR + 1])
        ld_k, ld_v = {}, {}
        for (s, h) in pair_order:
            p = 2 * s + h
            g = 2 * slot_dev[s] + h
            ld_k[(s, h)] = pltpu.make_async_copy(kt_hbm.at[pl.ds(B_LOC * me, B_LOC), g], k_v.at[p], ksem.at[p])
            ld_v[(s, h)] = pltpu.make_async_copy(vt_hbm.at[pl.ds(B_LOC * me, B_LOC), g], v_v.at[p], vsem.at[p])

        early = [me >= 2, (me == 1) | (me == 2)]
        bar = pltpu.get_barrier_semaphore()

        ld_wq[0].start()
        for d, pos in ((1, 1), (0, 3)):
            @pl.when(me == pos)
            def _():
                pl.semaphore_signal(bar, inc=1, device_id=(2,), device_id_type=MESH)
                pl.semaphore_wait(bar, 1)
                cp[d][("hd", 0)].start()
                pl.semaphore_signal(rdy.at[1 - d], inc=1, device_id=(0,), device_id_type=MESH)

        @pl.when(me == 0)
        def _():
            pl.semaphore_signal(bar, inc=1, device_id=(1,), device_id_type=MESH)
            pl.semaphore_signal(bar, inc=1, device_id=(3,), device_id_type=MESH)

        for ld in ld_wq[1:] + [ld_x, ld_wo]:
            fence()
            ld.start()
        for sh in pair_order:
            fence()
            ld_k[sh].start()
            ld_v[sh].start()

        @pl.when(me == 2)
        def _():
            pl.semaphore_wait(bar, 2)
            cp[0][("hd", 0)].start()
            cp[1][("hd", 0)].start()
            pl.semaphore_signal(rdy.at[1], inc=1, device_id=(3,), device_id_type=MESH)
            pl.semaphore_signal(rdy.at[0], inc=1, device_id=(1,), device_id_type=MESH)

        for i in range(NR):
            ld_wq[i].wait()
            for h in range(2):
                w_all[0, 512 * h + roff[i]:512 * h + roff[i] + lrows[i], :] = (
                    wq_f[roff[i]:roff[i] + lrows[i], 128 * h:128 * (h + 1)].astype(bf16))
            for d in range(2):
                @pl.when(early[d])
                def _():
                    cp[d][("qa", i)].start()
                    if i == NR - 1:
                        cp[d][("qb", 0)].start()
        for d in range(2):
            @pl.when(jnp.logical_not(early[d]))
            def _():
                pl.semaphore_wait(rdy.at[d], 1)
                for i in range(NR):
                    cp[d][("qa", i)].start()
                cp[d][("hd", 0)].start()
                cp[d][("qb", 0)].start()

        ld_x.wait()
        x_b[...] = x_f[...].astype(bf16)
        ld_wo.wait()
        for par in range(2):
            for c in range(4):
                for hh in range(2):
                    h = 2 * hh + par
                    w_all[0, _wo_row(par, c, hh):_wo_row(par, c, hh) + 64, :] = (
                        wo_f[64 * h:64 * (h + 1), 128 * c:128 * (c + 1)].astype(bf16))
        cp[0][("oa", 0)].start()
        cp[1][("oa", 0)].start()

        lo = lax.broadcasted_iota(jnp.int32, (T, 128), 1) < BLK
        m_diag = ((lax.broadcasted_iota(jnp.int32, (128, 128), 0) < BLK)
                  == (lax.broadcasted_iota(jnp.int32, (128, 128), 1) < BLK))
        seg_sum = (jnp.where(m_diag, 1.0, 0.0).astype(bf16), jnp.where(m_diag, 0.0, 1.0).astype(bf16))
        lo_ctx = lo == ((lax.broadcasted_iota(jnp.int32, (T, 128), 0) & BLK) == 0)
        masked_keys = jnp.where(lax.broadcasted_iota(jnp.int32, (16, SQ), 0) * BLK
                                == (lax.broadcasted_iota(jnp.int32, (16, SQ), 1) & -BLK), 0.0, 1.0).astype(bf16)

        def block_weights(w):
            w = jnp.concatenate([w[0:BLK], pltpu.roll(w[BLK:128], BLK, 1)], axis=0)
            return jnp.where(m_diag, w, 0.0).astype(bf16), jnp.where(m_diag, 0.0, w).astype(bf16)

        def attn(pairs):
            for sh in pairs:
                ld_k[sh].wait()
                ld_v[sh].wait()
            qs = []
            for (s, h) in pairs:
                q = jnp.dot(x_b[...], w_all[s, 512 * h:512 * (h + 1), :], preferred_element_type=f32)
                qs.append((q * QSCALE).astype(bf16))
            scores = []
            for (s, h), q in zip(pairs, qs):
                blocks = []
                for b in range(B_LOC):
                    for t in range(2):
                        wk = block_weights(k_v[2 * s + h, b, :, 128 * t:128 * (t + 1)])
                        for j in range(2):
                            r0 = b * SQ + t * 128 + j * BLK
                            blocks.append(jnp.dot(q[r0:r0 + BLK], wk[j], preferred_element_type=f32))
                scores.append(jnp.concatenate(blocks, axis=0))
            probs = []
            for sc in scores:
                m0 = jnp.max(jnp.where(lo, sc, -jnp.inf), axis=1, keepdims=True)
                m1 = jnp.max(jnp.where(lo, -jnp.inf, sc), axis=1, keepdims=True)
                probs.append((jnp.exp2(sc - jnp.maximum(jnp.where(lo, m0, m1), MASKED)).astype(bf16),
                              jnp.exp2(jnp.minimum(MASKED - jnp.where(lo_ctx, m0, m1), 0.0))))
            for (s, h), (pe, pm) in zip(pairs, probs):
                p = 2 * s + h
                for b in range(B_LOC):
                    v_masked = lax.dot_general(masked_keys, v_v[p, b].astype(bf16), (((1,), (1,)), ((), ())),
                                               preferred_element_type=f32)
                    for t in range(2):
                        wv = block_weights(v_v[p, b, :, 128 * t:128 * (t + 1)])
                        for j in range(2):
                            r0 = b * SQ + t * 128 + j * BLK
                            pb = pe[r0:r0 + BLK]
                            l = jnp.dot(pb, seg_sum[j], preferred_element_type=f32)
                            o = lax.dot_general(pb, wv[j], (((1,), (1,)), ((), ())),
                                                preferred_element_type=f32)
                            l = l + (SQ - BLK) * pm[r0:r0 + BLK]
                            o = o + pm[r0:r0 + BLK] * v_masked[2 * t + j:2 * t + j + 1]
                            ctx[r0:r0 + BLK, 128 * p:128 * (p + 1)] = (o / l).astype(bf16)

        def oproj(pairs, c, first=False, msplit=1):
            m = T // msplit
            for mi in range(msplit):
                rows = slice(mi * m, (mi + 1) * m)
                acc = None
                for (s, hh) in pairs:
                    p = 2 * s + hh
                    w = jnp.concatenate([w_all[s, _wo_row(par, c, hh):_wo_row(par, c, hh) + 64, :]
                                         for par in range(2)], axis=0)
                    d = jnp.dot(ctx[rows, 128 * p:128 * (p + 1)], w, preferred_element_type=f32)
                    acc = d if acc is None else acc + d
                if first:
                    out_ref[rows, 128 * c:128 * (c + 1)] = acc
                else:
                    out_ref[rows, 128 * c:128 * (c + 1)] += acc

        attn(pair_order[0:2])
        for d in range(2):
            cp[d][("hd", 0)].wait_recv()
            w_all[1 + d, 512 * d + F0:512 * d + DM, :] = head_f[d].astype(bf16)
            for i in range(NR):
                cp[d][("qa", i)].wait_recv()
            cp[d][("fq", 0)].start()
            cp[d][("ob", 0)].start()
            cp[d][("ob", 1)].start()
        attn(pair_order[2:4])
        wait_recv("qb")
        attn(pair_order[4:6])
        for c in range(4):
            oproj([(0, 0), (0, 1)], c, first=True)
        for d in range(2):
            cp[d][("oa", 0)].wait_recv()
            for i in range(NF):
                cp[d][("fo", i)].start()
        pl.semaphore_wait(fsem, n_fence[0])
        wait_send("hd")
        for i in range(NR):
            wait_send("qa", i)
        wait_send("qb")
        wait_send("oa")
        wait_recv("fq")
        attn(pair_order[6:8])
        for i in range(2):
            wait_recv("ob", i)
            for c in (2 * i, 2 * i + 1):
                oproj([(1, 0), (1, 1), (2, 0), (2, 1)], c)
        wait_send("fq")
        wait_send("ob", 0)
        wait_send("ob", 1)
        for i in range(NF):
            wait_send("fo", i)
            wait_recv("fo", i)
            if i < 3:
                oproj([(3, 0), (3, 1)], i, msplit=2)
            else:
                oproj([(3, i - 3)], 3, msplit=4)

    out = pl.pallas_call(
        body,
        out_shape=jax.ShapeDtypeStruct((T, DM), f32),
        in_specs=[pl.BlockSpec(memory_space=pl.ANY)] * 5,
        out_specs=pl.BlockSpec(memory_space=pltpu.VMEM),
        scratch_shapes=[
            pltpu.VMEM((T, DM), f32),
            pltpu.VMEM((T, DM), bf16),
            pltpu.VMEM((DM, 256), f32),
            pltpu.VMEM((256, DM), f32),
            pltpu.VMEM((4, 2048, 128), bf16),
            pltpu.VMEM((2, F32ROWS, 128), f32),
            pltpu.VMEM((8, B_LOC, 128, SQ), f32),
            pltpu.VMEM((8, B_LOC, 128, SQ), f32),
            pltpu.VMEM((T, 1024), bf16),
            pltpu.SemaphoreType.DMA((NR + 2,)),
            pltpu.SemaphoreType.DMA((8,)),
            pltpu.SemaphoreType.DMA((8,)),
            pltpu.SemaphoreType.DMA((2 * NP,)),
            pltpu.SemaphoreType.DMA((2 * NP,)),
            pltpu.SemaphoreType.REGULAR,
            pltpu.SemaphoreType.REGULAR((2,)),
        ],
        compiler_params=pltpu.CompilerParams(collective_id=0, disable_semaphore_checks=True,
                                             vmem_limit_bytes=32 * 1024 * 1024),
    )(x2, Wq, kt, vt, Wo)
    return out.reshape(B_LOC, SQ, DM)
```
